```python
import numpy as np

kernel_name = "dist_rope_attn_qseq_b2_sq128_d512_hq4_dh64"

def setup_inputs():
    x = np.random.randn(2, 512, 512).astype(np.float32)
    Wq = np.random.randn(512, 256).astype(np.float32) * 0.02
    Wk = np.random.randn(512, 256).astype(np.float32) * 0.02
    Wv = np.random.randn(512, 256).astype(np.float32) * 0.02
    Wo = np.random.randn(256, 512).astype(np.float32) * 0.02
    return {"x": x, "Wq": Wq, "Wk": Wk, "Wv": Wv, "Wo": Wo}

def reference(x, Wq, Wk, Wv, Wo):
    B, Sq, Hq, Dh = 2, 512, 4, 64
    inv = 1.0 / (10000.0 ** (np.arange(0, Dh, 2) / Dh))
    pos = np.arange(Sq)[:, None] * inv[None, :]
    cos = np.repeat(np.cos(pos), 2, axis=-1).astype(np.float32)
    sin = np.repeat(np.sin(pos), 2, axis=-1).astype(np.float32)
    def rot(t):
        t2 = t.reshape(B, Sq, Hq, Dh // 2, 2)
        t_r = np.stack([-t2[..., 1], t2[..., 0]], axis=-1).reshape(B, Sq, Hq, Dh)
        return t * cos[None, :, None, :] + t_r * sin[None, :, None, :]
    Q = rot((x @ Wq).reshape(B, Sq, Hq, Dh))
    K = rot((x @ Wk).reshape(B, Sq, Hq, Dh))
    V = (x @ Wv).reshape(B, Sq, Hq, Dh)
    s = np.einsum('bihd,bjhd->bhij', Q, K).astype(np.float32) * 0.125
    s_max = s.max(axis=-1, keepdims=True)
    w = np.exp(s - s_max)
    w = w / w.sum(axis=-1, keepdims=True)
    ctx = np.einsum('bhij,bjhd->bihd', w, V).reshape(B, Sq, Hq * Dh)
    return ctx @ Wo
```

```python
import functools
import numpy as np
import jax
import jax.numpy as jnp
from jax import lax
from jax.experimental import pallas as pl
from jax.experimental.pallas import tpu as pltpu

B, SQ, D, HD, NH, DH = 2, 128, 512, 256, 4, 64
LOG2E = 1.4426950408889634
QSCALE = 0.125 * LOG2E

f32, bf16 = jnp.float32, jnp.bfloat16
NT = (((1,), (1,)), ((), ()))
TN = (((0,), (0,)), ((), ()))
NN = (((1,), (0,)), ((), ()))


def _body(x_ref, wq_ref, wk_ref, wv_ref, wo_ref, out_ref,
          xf, wqf, wkf, wvf, wof,
          kbuf, vtbuf, qbuf, psend, precv, own_o, own_st, outbuf,
          lsem, ssem, rsem, osem):
    me = lax.axis_index("i")
    pa = me ^ 1
    pb = 3 - me
    kvp = (pa, pb)
    qp = (pb, pa)

    bsem = pltpu.get_barrier_semaphore()
    pl.semaphore_signal(bsem, inc=1, device_id=(pa,), device_id_type=pl.DeviceIdType.MESH)
    pl.semaphore_signal(bsem, inc=1, device_id=(pb,), device_id_type=pl.DeviceIdType.MESH)

    ld = {}
    def load(name, src, dst, i):
        c = pltpu.make_async_copy(src, dst, lsem.at[i])
        c.start()
        ld[name] = c
    load("x0", x_ref.at[0], xf.at[0], 0)
    load("wk", wk_ref, wkf, 1)
    load("wv", wv_ref, wvf, 2)
    load("x1", x_ref.at[1], xf.at[1], 3)
    load("wq", wq_ref, wqf, 4)
    load("wo", wo_ref, wof, 5)

    def rcopy(src, dst, slot, dev):
        return pltpu.make_async_remote_copy(src_ref=src, dst_ref=dst, send_sem=ssem.at[slot], recv_sem=rsem.at[slot],
                                            device_id=(dev,), device_id_type=pl.DeviceIdType.MESH)
    def kcopy(b, hp):
        return rcopy(kbuf.at[b, hp, 0], kbuf.at[b, hp, 1], 0 + b * 2 + hp, kvp[hp])
    def vcopy(b, hp):
        return rcopy(vtbuf.at[b, hp, 0], vtbuf.at[b, hp, 1], 4 + b * 2 + hp, kvp[hp])
    def qcopy(b, hp):
        return rcopy(qbuf.at[b, hp, 0], qbuf.at[b, hp, 1], 8 + b * 2 + hp, qp[hp])
    def pcopy(b, hp):
        return rcopy(psend.at[b, hp], precv.at[b, hp], 12 + b * 2 + hp, qp[hp])

    lane = lax.broadcasted_iota(jnp.int32, (SQ, 128), 1)
    row = lax.broadcasted_iota(jnp.int32, (SQ, 128), 0)
    fi = ((lane % DH) // 2).astype(f32)
    inv = jnp.exp2(fi * (-2.0 / DH * np.log2(10000.0)))
    ang = (row + me * SQ).astype(f32) * inv
    even = (lane % 2) == 0
    cos = jnp.cos(ang)
    sin = jnp.sin(ang)
    sin = jnp.where(even, -sin, sin)

    def rope(t, c, s):
        a = pltpu.roll(t, 127, 1)
        bb = pltpu.roll(t, 1, 1)
        return t * c + jnp.where(even, a, bb) * s

    pl.semaphore_wait(bsem, 2)

    def kv_block(b, xb):
        if b == 0:
            ld["wk"].wait()
        k = lax.dot_general(xb, wkf[...].astype(bf16), NN, preferred_element_type=f32)
        for hp in range(2):
            kbuf[b, hp, 0] = rope(k[:, hp * 128:(hp + 1) * 128], cos, sin).astype(bf16)
            kcopy(b, hp).start()
        if b == 0:
            ld["wv"].wait()
        v = lax.dot_general(xb, wvf[...].astype(bf16), NN, preferred_element_type=f32)
        for hp in range(2):
            vtbuf[b, hp, 0] = v[:, hp * 128:(hp + 1) * 128].T.astype(bf16)
            vcopy(b, hp).start()

    ld["x0"].wait()
    xb0 = xf[0].astype(bf16)
    kv_block(0, xb0)
    ld["x1"].wait()
    xb1 = xf[1].astype(bf16)
    kv_block(1, xb1)
    ld["wq"].wait()
    wqb = wqf[...].astype(bf16)
    cq = cos * QSCALE
    sq = sin * QSCALE
    for b, xb in ((0, xb0), (1, xb1)):
        q = lax.dot_general(xb, wqb, NN, preferred_element_type=f32)
        for hp in range(2):
            qbuf[b, hp, 0] = rope(q[:, hp * 128:(hp + 1) * 128], cq, sq).astype(bf16)
            qcopy(b, hp).start()

    lane_q = lax.broadcasted_iota(jnp.int32, (SQ, 128), 1)
    sub8 = lax.broadcasted_iota(jnp.int32, (8, 128), 0)

    def attn(b, hp, src):
        q = qbuf[b, hp, src]
        k = kbuf[b, hp].reshape(256, 128)
        vt = jnp.concatenate([vtbuf[b, hp, 0], vtbuf[b, hp, 1]], axis=1)
        outs = []
        st = jnp.zeros((8, 128), f32)
        for h in range(2):
            qm = jnp.where((lane_q // DH) == h, q, jnp.zeros_like(q))
            s = lax.dot_general(k, qm, NT, preferred_element_type=f32)
            m = jnp.max(s, axis=0, keepdims=True)
            p = jnp.exp2(s - m)
            l = jnp.sum(p, axis=0, keepdims=True)
            o = lax.dot_general(vt[h * DH:(h + 1) * DH], p.astype(bf16), NN, preferred_element_type=f32)
            outs.append(o)
            st = jnp.where(sub8 == 2 * h, m, st)
            st = jnp.where(sub8 == 2 * h + 1, l, st)
        return jnp.concatenate(outs, axis=0), st

    def own_attn(b, hp):
        o, st = attn(b, hp, 0)
        own_o[b, hp] = o
        own_st[b, hp] = st

    def ptn_attn(b, hp):
        o, st = attn(b, hp, 1)
        psend[b, hp, 0:128] = o.astype(bf16)
        psend[b, hp, 128:144] = pltpu.bitcast(st, bf16)
        pcopy(b, hp).start()

    for b in range(2):
        for hp in range(2):
            kcopy(b, hp).wait_recv()
            vcopy(b, hp).wait_recv()
            own_attn(b, hp)
    for b in range(2):
        for hp in range(2):
            qcopy(b, hp).wait_recv()
            ptn_attn(b, hp)

    ld["wo"].wait()
    wob = wof[...].astype(bf16)
    subf = lax.broadcasted_iota(jnp.int32, (128, 128), 0)
    ocps = []
    for b in range(2):
        ctx = []
        for hp in range(2):
            pcopy(b, hp).wait_recv()
            o1 = own_o[b, hp]
            s1 = own_st[b, hp]
            o2 = precv[b, hp, 0:128].astype(f32)
            s2 = pltpu.bitcast(precv[b, hp, 128:144], f32)
            hs = []
            for h in range(2):
                m1, l1 = s1[2 * h:2 * h + 1], s1[2 * h + 1:2 * h + 2]
                m2, l2 = s2[2 * h:2 * h + 1], s2[2 * h + 1:2 * h + 2]
                M = jnp.maximum(m1, m2)
                a1 = jnp.exp2(m1 - M)
                a2 = jnp.exp2(m2 - M)
                r = 1.0 / (a1 * l1 + a2 * l2)
                hs.append((a1 * r) * o1[h * DH:(h + 1) * DH] + (a2 * r) * o2[h * DH:(h + 1) * DH])
            ctx.append(jnp.concatenate(hs, axis=0).astype(bf16))
        ct = jnp.concatenate(ctx, axis=0)
        outbuf[b] = lax.dot_general(ct, wob, TN, preferred_element_type=f32)
        c = pltpu.make_async_copy(outbuf.at[b], out_ref.at[b], osem.at[b])
        c.start()
        ocps.append(c)
    for b in range(2):
        for hp in range(2):
            kcopy(b, hp).wait_send()
            vcopy(b, hp).wait_send()
            qcopy(b, hp).wait_send()
            pcopy(b, hp).wait_send()
    for c in ocps:
        c.wait()


def pallas_dist_rope_attn_qseq_b2_sq128_d512_hq4_dh64_kernel(x, Wq, Wk, Wv, Wo):
    ANY = pl.BlockSpec(memory_space=pl.ANY)
    return pl.pallas_call(
        _body,
        out_shape=jax.ShapeDtypeStruct((B, SQ, D), f32),
        in_specs=[ANY] * 5,
        out_specs=ANY,
        scratch_shapes=[
            pltpu.VMEM((B, SQ, D), f32),
            pltpu.VMEM((D, HD), f32), pltpu.VMEM((D, HD), f32), pltpu.VMEM((D, HD), f32), pltpu.VMEM((HD, D), f32),
            pltpu.VMEM((B, 2, 2, SQ, 128), bf16),
            pltpu.VMEM((B, 2, 2, 128, SQ), bf16),
            pltpu.VMEM((B, 2, 2, SQ, 128), bf16),
            pltpu.VMEM((B, 2, 144, 128), bf16),
            pltpu.VMEM((B, 2, 144, 128), bf16),
            pltpu.VMEM((B, 2, 128, 128), f32),
            pltpu.VMEM((B, 2, 8, 128), f32),
            pltpu.VMEM((B, SQ, D), f32),
            pltpu.SemaphoreType.DMA((6,)),
            pltpu.SemaphoreType.DMA((16,)),
            pltpu.SemaphoreType.DMA((16,)),
            pltpu.SemaphoreType.DMA((2,)),
        ],
        compiler_params=pltpu.CompilerParams(collective_id=0, vmem_limit_bytes=64 * 1024 * 1024),
    )(x, Wq, Wk, Wv, Wo)
```

```python
import numpy as np
import jax
import jax.numpy as jnp
from jax import lax
from jax.experimental import pallas as pl
from jax.experimental.pallas import tpu as pltpu

B, SQ, D, HD, NH, DH = 2, 128, 512, 256, 4, 64
LOG2E = 1.4426950408889634
QSCALE = 0.125 * LOG2E
INV_FREQ = [float(v) for v in 1.0 / (10000.0 ** (np.arange(0, DH, 2) / DH))]

f32, bf16, u32, i32 = jnp.float32, jnp.bfloat16, jnp.uint32, jnp.int32
NT = (((1,), (1,)), ((), ()))
TN = (((0,), (0,)), ((), ()))
NN = (((1,), (0,)), ((), ()))
MESH = pl.DeviceIdType.MESH


def pk(v):
    return pltpu.bitcast(v.astype(bf16), u32)


def up(u):
    return pltpu.bitcast(u, bf16)


LOADS = {"x0a": 0, "x1a": 1, "wk0": 2, "wk1": 3, "wv0": 4, "wv1": 5, "wq0": 6, "wq1": 7, "wo": 8, "x0b": 9, "x1b": 10}


def parse_tiles(s):
    return [(t[0], int(t[1]), int(t[2]), (0, 1) if len(t) == 3 else ("ab".index(t[3]),)) for t in s.split(",")]


def expand(loads, tasks):
    steps = ["ld:" + ",".join(loads), "tables"]
    waited = set()

    def need_load(n):
        if n not in waited:
            waited.add(n)
            steps.append("w:" + n)

    def need_recv(kind, b, hp, h=0):
        key = "r:%s:%d:%d:%d" % (kind, b, hp, h)
        if key not in waited:
            waited.add(key)
            steps.append(key)

    def need_bar():
        if "barrier" not in waited:
            waited.add("barrier")
            steps.append("barrier")

    casted = set()
    for i_task, t in enumerate(tasks):
        a = t.split(":")
        if a[0] in ("K", "V", "Q"):
            toks = a[1].split(",")
            for x in toks:
                for half in (x[2] if len(x) == 3 else "ab"):
                    key = x[0] + half
                    if key not in casted:
                        need_load("x" + key)
                        steps.append("cast:" + key)
                        casted.add(key)
            for x in toks:
                need_load("w%s%s" % (a[0].lower(), x[1]))
            steps.append(t)
            need_bar()
            steps.append("send:%s:%s" % (a[0].lower(), ",".join(
                x[:2] + h for x in toks for h in ("01" if len(x) == 2 else str("ab".index(x[2]))))))
        elif a[0] in ("A", "SE", "PV"):
            for src, b, hp, hs in parse_tiles(a[1]):
                if a[0] in ("A", "SE"):
                    need_recv("k", b, hp, 0)
                    need_recv("k", b, hp, 1)
                    if src == "p":
                        need_recv("q", b, hp, 0)
                        need_recv("q", b, hp, 1)
                if a[0] in ("A", "PV"):
                    for h in hs:
                        need_recv("v", b, hp, h)
            steps.append(t)
            pt = ["%d%d%d" % (b, hp, h) for src, b, hp, hs in parse_tiles(a[1]) if src == "p" for h in hs]
            if a[0] in ("A", "PV") and pt:
                steps.append("send:p:" + ",".join(pt))
        elif a[0] == "F":
            if i_task == len(tasks) - 1:
                steps.append("waitsend")
            need_load("wo")
            b = int(a[1])
            for x in a[2].split(","):
                need_recv("p", b, int(x[0]), 0)
                need_recv("p", b, int(x[0]), "ab".index(x[1]))
            steps.append(t)
        else:
            raise ValueError(t)
    return steps


def make_body(progs):
    def body(x_ref, wq_ref, wk_ref, wv_ref, wo_ref, out_ref,
             xf, xb, wqf, wkf, wvf, wof, tab,
             kbuf, vtbuf, qbuf, sbuf, pbuf, psend, precv, own_o, own_st,
             lsem, ssem, rsem):
        me = lax.axis_index("i")
        pa = me ^ 1
        pb = 3 - me
        kvp = (pa, pb)
        qp = (pb, pa)

        bsem = pltpu.get_barrier_semaphore()
        pl.semaphore_signal(bsem, inc=1, device_id=(pa,), device_id_type=MESH)
        pl.semaphore_signal(bsem, inc=1, device_id=(pb,), device_id_type=MESH)

        def lcopy(name, flip=0):
            i = LOADS[name]
            if name[0] == "x":
                b, rows = int(name[1]), pl.ds(64 * "ab".index(name[2]), 64)
                return pltpu.make_async_copy(x_ref.at[b, rows], xf.at[b, rows], lsem.at[i])
            if name == "wo":
                return pltpu.make_async_copy(wo_ref, wof, lsem.at[i])
            hp = int(name[2]) ^ flip
            src, dst = {"k": (wk_ref, wkf), "v": (wv_ref, wvf), "q": (wq_ref, wqf)}[name[1]]
            off = hp * 128 if isinstance(hp, int) else pl.multiple_of(hp * 128, 128)
            return pltpu.make_async_copy(src.at[:, pl.ds(off, 128)], dst.at[hp], lsem.at[i])

        def rcopy(kind, b, hp, h):
            slot = {"k": 0, "q": 8, "v": 16, "p": 24}[kind] + 4 * b + 2 * hp + h
            devs = kvp if kind in "kv" else qp
            dev = devs[hp] if isinstance(hp, int) else jnp.where(hp == 0, devs[0], devs[1])
            if kind == "p":
                rows = pl.ds(0, 36) if h == 0 else pl.ds(40, 32)
                src, dst = psend.at[b, hp, rows], precv.at[b, hp, rows]
            else:
                buf = {"k": kbuf, "q": qbuf, "v": vtbuf}[kind]
                src, dst = buf.at[b, hp, 0, pl.ds(32 * h, 32)], buf.at[b, hp, 1, pl.ds(32 * h, 32)]
            return pltpu.make_async_remote_copy(src_ref=src, dst_ref=dst, send_sem=ssem.at[slot], recv_sem=rsem.at[slot],
                                                device_id=(dev,), device_id_type=MESH)

        def rope(t, c, s):
            lane = lax.broadcasted_iota(i32, t.shape, 1)
            a = pltpu.roll(t, 127, 1)
            bb = pltpu.roll(t, 1, 1)
            return t * c + jnp.where((lane & 1) == 0, a, bb) * s

        def do_tables():
            lane1 = lax.broadcasted_iota(i32, (8, 128), 1)
            fi = (lane1 & (DH - 1)) >> 1
            inv8 = jnp.zeros((8, 128), f32)
            for i, v in enumerate(INV_FREQ):
                inv8 = jnp.where(fi == i, v, inv8)
            inv = jnp.concatenate([inv8] * (SQ // 8), axis=0)
            lane = lax.broadcasted_iota(i32, (SQ, 128), 1)
            row = lax.broadcasted_iota(i32, (SQ, 128), 0)
            ang = (row + me * SQ).astype(f32) * inv
            cos = jnp.cos(ang)
            sin = jnp.sin(ang)
            sin = jnp.where((lane & 1) == 0, -sin, sin)
            tab[0] = cos
            tab[1] = sin
            tab[2] = cos * QSCALE
            tab[3] = sin * QSCALE

        def proj(xv, w_ref):
            return lax.dot_general(xv, w_ref[...].astype(bf16), NN, preferred_element_type=f32)

        def do_S(src, b, hp):
            lane64 = lax.broadcasted_iota(i32, (64, 128), 1)
            q = qbuf[b, hp, src]
            for h in range(2):
                qm = up(jnp.where((lane64 >> 6) == h, q, jnp.zeros_like(q)))
                for half in range(2):
                    sbuf[src, b, hp, h, half * 128:(half + 1) * 128] = lax.dot_general(
                        up(kbuf[b, hp, half]), qm, NT, preferred_element_type=f32)

        def softmax_parts(src, b, hp):
            sub8 = lax.broadcasted_iota(i32, (4, 128), 0)
            st = jnp.zeros((4, 128), f32)
            ps = []
            for h in range(2):
                s = sbuf[src, b, hp, h]
                m = jnp.max(s, axis=0, keepdims=True)
                p = jnp.exp2(s - m)
                l = jnp.sum(p, axis=0, keepdims=True)
                ps.append(p.astype(bf16))
                st = jnp.where(sub8 == 2 * h, m, st)
                st = jnp.where(sub8 == 2 * h + 1, l, st)
            return ps, st

        def pv(b, hp, h, p):
            vt = up(jnp.concatenate([vtbuf[b, hp, 0, h * 32:(h + 1) * 32], vtbuf[b, hp, 1, h * 32:(h + 1) * 32]], axis=1))
            return lax.dot_general(vt, p, NN, preferred_element_type=f32)

        def put_o(src, b, hp, h, o):
            if src == 0:
                own_o[b, hp, h * DH:(h + 1) * DH] = o
            else:
                psend[b, hp, 40 * h:40 * h + 32] = pk(o)

        def put_st(src, b, hp, st):
            if src == 0:
                own_st[b, hp] = st
            else:
                psend[b, hp, 32:36] = pltpu.bitcast(st, u32)

        def do_X(src, b, hp, hs):
            ps, st = softmax_parts(src, b, hp)
            for h in range(2):
                put_o(src, b, hp, h, pv(b, hp, h, ps[h]))
            put_st(src, b, hp, st)

        def do_E(src, b, hp, hs):
            ps, st = softmax_parts(src, b, hp)
            for h in range(2):
                pbuf[src, b, hp, h] = pltpu.bitcast(ps[h], u32)
            put_st(src, b, hp, st)

        def do_PV(src, b, hp, hs):
            for h in hs:
                put_o(src, b, hp, h, pv(b, hp, h, up(pbuf[src, b, hp, h])))

        def merged(b, hp, h):
            o1 = own_o[b, hp, h * DH:(h + 1) * DH]
            s1 = own_st[b, hp]
            o2 = up(precv[b, hp, 40 * h:40 * h + 32]).astype(f32)
            s2 = pltpu.bitcast(precv[b, hp, 32:36], f32)
            m1, l1 = s1[2 * h:2 * h + 1], s1[2 * h + 1:2 * h + 2]
            m2, l2 = s2[2 * h:2 * h + 1], s2[2 * h + 1:2 * h + 2]
            M = jnp.maximum(m1, m2)
            a1 = jnp.exp2(m1 - M)
            a2 = jnp.exp2(m2 - M)
            r = 1.0 / (a1 * l1 + a2 * l2)
            return ((a1 * r) * o1 + (a2 * r) * o2).astype(bf16)

        def do_F(b, heads, first):
            ct = jnp.concatenate([merged(b, hp, h) for hp, h in heads], axis=0)
            ws = []
            for hp, h in heads:
                off = hp * 128 + h * DH
                ws.append(wof[pl.ds(off if isinstance(off, int) else pl.multiple_of(off, DH), DH)])
            w = jnp.concatenate(ws, axis=0)
            r = lax.dot_general(ct, w.astype(bf16), TN, preferred_element_type=f32)
            if first:
                out_ref[b] = r
            else:
                out_ref[b] += r

        def run_prog(steps, flip=0):
            seenF = set()

            def run(st):
                a = st.split(":")
                op = a[0]
                if op == "ld":
                    for n in a[1].split(","):
                        lcopy(n, flip).start()
                elif op == "w":
                    lcopy(a[1], flip).wait()
                elif op == "barrier":
                    pl.semaphore_wait(bsem, 2)
                elif op == "waitsend":
                    for b in range(2):
                        for hp in range(2):
                            for kind in "kvqp":
                                for h in range(2):
                                    rcopy(kind, b, hp, h).wait_send()
                elif op == "cast":
                    b, h = int(a[1][0]), "ab".index(a[1][1])
                    xb[b, 32 * h:32 * h + 32] = pk(xf[b, 64 * h:64 * h + 64])
                elif op in ("K", "V", "Q"):
                    for x in a[1].split(","):
                        b, hp = int(x[0]), int(x[1]) ^ flip
                        r0, n = (0, 128) if len(x) == 2 else (64 * "ab".index(x[2]), 64)
                        rows, prow = slice(r0, r0 + n), slice(r0 // 2, (r0 + n) // 2)
                        xv = up(xb[b, prow])
                        if op == "K":
                            kbuf[b, hp, 0, prow] = pk(rope(proj(xv, wkf.at[hp]), tab[0, rows], tab[1, rows]))
                        elif op == "Q":
                            qbuf[b, hp, 0, prow] = pk(rope(proj(xv, wqf.at[hp]), tab[2, rows], tab[3, rows]))
                        else:
                            vtbuf[b, hp, 0] = pltpu.bitcast(proj(xv, wvf.at[hp]).astype(bf16).T, u32)
                elif op == "send":
                    for x in a[2].split(","):
                        rcopy(a[1], int(x[0]), int(x[1]) ^ flip, int(x[2])).start()
                elif op == "r":
                    rcopy(a[1], int(a[2]), int(a[3]) ^ flip, int(a[4])).wait_recv()
                elif op in ("A", "SE", "PV"):
                    tiles = [(0 if s == "o" else 1, b, hp ^ flip, hs) for s, b, hp, hs in parse_tiles(a[1])]
                    if op in ("A", "SE"):
                        for t in tiles:
                            do_S(*t[:3])
                    for t in tiles:
                        {"A": do_X, "SE": do_E, "PV": do_PV}[op](*t)
                elif op == "F":
                    b = int(a[1])
                    do_F(b, [(int(x[0]) ^ flip, "ab".index(x[1])) for x in a[2].split(",")], b not in seenF)
                    seenF.add(b)
                else:
                    raise ValueError(st)

            for st in steps:
                run(st)

        prog_f, prog_m, prog_l = progs
        flip = (me == 1).astype(i32)
        role = jnp.where(me == 0, 0, jnp.where(me == 2, 2, 1))
        lax.switch(role, [lambda: run_prog(prog_f[:1]), lambda: run_prog(prog_m[:1], flip), lambda: run_prog(prog_l[:1])])
        do_tables()
        lax.switch(role, [lambda: run_prog(prog_f[2:]), lambda: run_prog(prog_m[2:], flip), lambda: run_prog(prog_l[2:])])

    return body


def make_kernel(progs):
    def kernel(x, Wq, Wk, Wv, Wo):
        HBM = pl.BlockSpec(memory_space=pltpu.HBM)
        return pl.pallas_call(
            make_body(progs),
            out_shape=pltpu.VMEM((B, SQ, D), f32),
            in_specs=[HBM] * 5,
            out_specs=pl.BlockSpec(memory_space=pltpu.VMEM),
            scratch_shapes=[
                pltpu.VMEM((B, SQ, D), f32),
                pltpu.VMEM((B, SQ // 2, D), u32),
                pltpu.VMEM((2, D, 128), f32), pltpu.VMEM((2, D, 128), f32), pltpu.VMEM((2, D, 128), f32),
                pltpu.VMEM((HD, D), f32),
                pltpu.VMEM((4, SQ, 128), f32),
                pltpu.VMEM((B, 2, 2, 64, 128), u32),
                pltpu.VMEM((B, 2, 2, 64, 128), u32),
                pltpu.VMEM((B, 2, 2, 64, 128), u32),
                pltpu.VMEM((2, B, 2, 2, 256, 128), f32),
                pltpu.VMEM((2, B, 2, 2, 128, 128), u32),
                pltpu.VMEM((B, 2, 72, 128), u32),
                pltpu.VMEM((B, 2, 72, 128), u32),
                pltpu.VMEM((B, 2, 128, 128), f32),
                pltpu.VMEM((B, 2, 4, 128), f32),
                pltpu.SemaphoreType.DMA((11,)),
                pltpu.SemaphoreType.DMA((32,)),
                pltpu.SemaphoreType.DMA((32,)),
            ],
            compiler_params=pltpu.CompilerParams(collective_id=0, vmem_limit_bytes=32 * 1024 * 1024,
                                                 disable_semaphore_checks=True, disable_bounds_checks=True),
        )(x, Wq, Wk, Wv, Wo)
    return kernel


SCHED_F = (
    "x1a x1b x0a x0b wq0 wq1 wk1 wk0 wv1 wv0 wo",
    "Q:10a,11,10b,00,01 K:01b,00b K:01a,00a,10,11 V:11 SE:p11 SE:o10 V:01,00,10 SE:p01 SE:p10 PV:p10,p11a SE:o01,o00,p00,o11 PV:p00a,p01a PV:o00b,p01b,o10a,o10b,p00b,o01a PV:o01b,o00a,o11b,p11b,o11a F:0:0a,0b,1a,1b F:1:0a,1a F:1:0b,1b")
SCHED_M = (
    "x1b wq0 x1a wk1 wk0 x0a x0b wq1 wv0 wv1 wo",
    "Q:10b Q:10a K:11b,11a K:10b K:01,10a K:00b,00a Q:00a,00b,01,11b V:11,00,01 Q:11a V:10 SE:p00 SE:o10 SE:o00 PV:p00b,p00a SE:o11,p10,o01 PV:p10 A:p01 SE:p11 PV:p11a PV:o11b,o00,o10b,o11a,p11b,o01b,o01a PV:o10a F:0:1a,0b,0a,1b F:1:1a,0a,1b,0b")
SCHED_L = (
    "x0b wk0 wk1 x0a x1a x1b wv0 wv1 wq1 wq0 wo",
    "K:00b K:01b K:01a,00a K:10,11a K:11b V:00,01 V:11,10 Q:01,00a,00b,10,11 SE:o10,o00 SE:p00,o01,o11 SE:p01 PV:p00b,p00a,p01,o00a SE:p10,p11 PV:p11a,p10a PV:o11b,o11a,o10,o00b,p10b,p11b,o01b PV:o01a F:0:1b,1a F:0:0b,0a F:1:0b,1b,0a,1a")


def pallas_dist_rope_attn_qseq_b2_sq128_d512_hq4_dh64_kernel(
    x: jax.Array,
    Wq: jax.Array,
    Wk: jax.Array,
    Wv: jax.Array,
    Wo: jax.Array,
):
    progs = tuple(expand(l.split(), t.split()) for l, t in (SCHED_F, SCHED_M, SCHED_L))
    return make_kernel(progs)(x, Wq, Wk, Wv, Wo)
```
